```python
import numpy as np

kernel_name = "dist_sparse_attn_strided_qseq_b1_sq1024_skv1024_hq8_dh128"

def setup_inputs():
    x = np.random.randn(1, 4096, 1024).astype(np.float32)
    Wq = np.random.randn(1024, 4096).astype(np.float32) * 0.02
    K_ext = np.random.randn(1, 1024, 32, 128).astype(np.float32)
    V_ext = np.random.randn(1, 1024, 32, 128).astype(np.float32)
    Wo = np.random.randn(4096, 1024).astype(np.float32) * 0.02
    return {"x": x, "Wq": Wq, "K_ext": K_ext, "V_ext": V_ext, "Wo": Wo}

def reference(x, Wq, K_ext, V_ext, Wo):
    B, Sq, Skv, Hq, Dh = 1, 4096, 1024, 32, 128
    Q = (x @ Wq).reshape(B, Sq, Hq, Dh)
    qb = (np.arange(Sq) // 64)[:, None]
    kb = (np.arange(Skv) // 64)[None, :]
    mask = (qb == kb) | ((kb % 4) == (qb % 4))
    scores = np.einsum('bihd,bjhd->bhij', Q, K_ext).astype(np.float32) * 0.08838834764831843
    scores = np.where(mask[None, None, :, :], scores, -1e9)
    scores_max = scores.max(axis=-1, keepdims=True)
    w = np.exp(scores - scores_max)
    row_keep = mask.any(axis=1)
    w_sum = np.where(row_keep[None, None, :, None], w.sum(axis=-1, keepdims=True), 1.0)
    w = w / w_sum
    w = np.where(row_keep[None, None, :, None], w, 0.0)
    ctx = np.einsum('bhij,bjhd->bihd', w, V_ext).reshape(B, Sq, Hq * Dh)
    return ctx @ Wo
```

```python
import jax
import jax.numpy as jnp
from jax import lax
from jax.experimental import pallas as pl
from jax.experimental.pallas import tpu as pltpu

BF16 = jnp.bfloat16
F32 = jnp.float32
Q_SCALE = 0.08838834764831843 * 1.4426950408889634

FIRST_KINDS = ("QX", "QW")
KINDS = ("S", "SJ", "OX", "OO", "A", "QJ")
N_PROJ = dict(S=4, SJ=4, QX=2, QW=2, QJ=2)
N_ATTN = dict(S=4, SJ=4, A=4)
ROW = 4

SCHEDULE = """
    QW1:01,00 QX1:10,11 QW2:02,12 QX2:20,21 QW3:03,13 QX6:22,23 QX3:30,31 A kv3
    QJ0:32,33 S:40,41,42,43 kv4 S:44,04,14,24 kv5 SJ1:34,45,05,50 kv6 S:51,52,53,54
    A SJ2:55,46,56,60 kv7 S:61,62,63,64 S:65,66,15,25 SJ3:35,47,57,70
    S:67,71,72,73 S:74,75,76,77 A OX0 S:07,17,27,37 OX1 S:06,16,26,36 A
    OX2 OO0 OX3 OO1
"""
ATTN_AT = (1, 2, 7)
SIDE_WORK = ("w0 w1|w2|w3||w4|w5|w6 w7", "x0 o0|x1|||x2 o1|x3",
             "x4 o2|x5|||x6 o3|x7", "o4 o5|o6|||o7")


def _schedule():
    table, queue, loaded, done, received = [], [], set(), set(), set()
    for token in SCHEDULE.split():
        if token[:2] == "kv":
            table[-1][1] |= int(token[2:]) << 4
            continue
        name, _, units = token.partition(":")
        kind = name.rstrip("0123456789.")
        args = [int(v) for v in name[len(kind):].split(".") if v]
        proj = [(int(u[0]), int(u[1])) for u in units.split(",") if u]
        assert len(proj) == N_PROJ.get(kind, 0) and not done & set(proj)
        done |= set(proj)
        if kind in ("QX", "QW"):
            assert proj[0][kind == "QW"] == args[0] % 4
        if kind in ("QJ", "SJ"):
            assert proj[0][1] != 4 + args[0] and all(u[0] != 4 + args[0] for u in proj[:3])
            received.add(args[0])
        attn = []
        for slot in range(max(N_ATTN.get(kind, 0), len(proj))):
            if slot < N_ATTN.get(kind, 0):
                ready = loaded | {len(loaded)} if len(loaded) >= 4 else loaded
                queue.sort(key=lambda u: (u[0] < 4 or u[1] not in ready, u[1], u[0]))
                attn.append(queue.pop(0))
            queue += proj[slot:slot + 1]
        pending = queue + [(r, p) for r in range(8) for p in range(8) if (r, p) not in done]
        assert not any(u[0] >= 4 for u in pending) or kind not in ("OX", "OO")
        assert not pending or kind != "OO"
        fresh = sorted({p for _, p in attn} - loaded)
        assert len(fresh) <= 1
        loaded |= set(fresh)
        head = (KINDS if kind in KINDS else FIRST_KINDS).index(kind) | sum(v << (4 * i + 4) for i, v in enumerate(args))
        table.append([head, fresh[0] + 1 if fresh else 0, _pack(proj), _pack(attn)])
    assert not queue and len(done) == 64 and len(received) == 4
    return table


def _switch(index, names, branches):
    def pick(lo, hi):
        if hi - lo == 1:
            branches[names[lo]]()
        else:
            mid = (lo + hi) // 2
            lax.cond(index < mid, lambda: pick(lo, mid), lambda: pick(mid, hi))

    assert len(names) == len(branches)
    pick(0, len(branches))


def _pack(units):
    word = 0
    for i, (chunk, pair) in enumerate(units):
        word |= (chunk | (pair << 3)) << (6 * i)
    return word


def _dot(a, b):
    return jnp.dot(a, b, preferred_element_type=F32)


def _lhs_terms(a11, a12, a21, a22):
    return (a11 + a22, a21 + a22, a11, a22, a11 + a12, a21 - a11, a12 - a22)


def _rhs_terms(b11, b12, b21, b22):
    return (b11 + b22, b11, b12 - b22, b21 - b11, b22, b11 + b12, b21 + b22)


def _lhs_term(j, block):
    if j in (2, 3):
        return block(0 if j == 2 else 3)
    return _lhs_terms(*[block(q).astype(F32) for q in range(4)])[j].astype(BF16)


def _rhs_term(j, block):
    if j in (1, 4):
        return block(0 if j == 1 else 3)
    return _rhs_terms(*[block(q).astype(F32) for q in range(4)])[j].astype(BF16)


def _strassen(prod, emit):
    m2, m4 = prod(1), prod(3)
    emit(0, 1, 0, m2 + m4)
    m3, m5 = prod(2), prod(4)
    emit(1, 0, 1, m3 + m5)
    m1, m6 = prod(0), prod(5)
    emit(2, 1, 1, m1 - m2 + m3 + m6)
    m7 = prod(6)
    emit(3, 0, 0, m1 + m4 - m5 + m7)


USES = ((1, ((1, 0, 1), (1, 1, -1))), (3, ((1, 0, 1), (0, 0, 1))), (2, ((0, 1, 1), (1, 1, 1))),
        (4, ((0, 1, 1), (0, 0, -1))), (0, ((0, 0, 1), (1, 1, 1))), (5, ((1, 1, 1),)),
        (6, ((0, 0, 1),)))


def _body(x_hbm, wq_hbm, k_hbm, v_hbm, wo_hbm, out_ref,
          xf, wf, wof, kvf,
          xs, xr, ws, wr, wos, wor, ps, pr,
          xc, wc, woc, qb, cc, acc, tab,
          x_sem, w_sem, wo_sem, kv_sem, first_sem,
          send_sem, xr_sem, wr_sem, wor_sem, pr_sem):
    me = lax.axis_index("i")
    peer_a = me ^ 1
    peer_b = 3 - me

    barrier = pltpu.get_barrier_semaphore()
    for peer in (peer_a, peer_b):
        pl.semaphore_signal(barrier, inc=1, device_id=(peer,),
                            device_id_type=pl.DeviceIdType.MESH)

    def x_load(r):
        return pltpu.make_async_copy(
            x_hbm.at[:, pl.ds(pl.multiple_of(r * 64, 64), 64), :], xf.at[r], x_sem.at[r])

    def col_load(src, dst, sem, c):
        return pltpu.make_async_copy(
            src.at[:, pl.ds(pl.multiple_of(c * 256, 256), 256)], dst.at[c], sem.at[c])

    def kv_start(p):
        head = jnp.where(p < 4, me, peer_b) * 8 + 2 * (p & 3)
        for i, src in enumerate((k_hbm, v_hbm)):
            for b in range(2):
                pltpu.make_async_copy(
                    src.at[:, head + b, :], kvf.at[p, 2 * i + b], kv_sem.at[p]).start()

    def kv_wait(p):
        pltpu.make_async_copy(kvf.at[p], kvf.at[p], kv_sem.at[p]).wait()

    def remote(src, dst, stream, recv_sem, peer):
        def make(i, part=None, sem=None):
            at = (i,) if part is None else (i, part)
            sem = i if sem is None else sem
            return pltpu.make_async_remote_copy(
                src.at[at], dst.at[at], send_sem.at[stream], recv_sem.at[sem],
                device_id=(peer,), device_id_type=pl.DeviceIdType.MESH)
        return make

    x_send = remote(xs, xr, 0, xr_sem, peer_a)
    w_send = remote(ws, wr, 1, wr_sem, peer_b)
    wo_send = remote(wos, wor, 2, wor_sem, peer_b)
    p_send = remote(ps, pr, 3, pr_sem, peer_a)
    lead, rest = pl.ds(0, 1), pl.ds(1, 3)

    def p_sends(c):
        return p_send(2 * c, lead, 8 + c), p_send(2 * c, rest), p_send(2 * c + 1)

    lo, hi, left, right = pl.ds(0, 512), pl.ds(512, 512), pl.ds(0, 128), pl.ds(128, 128)
    first = [pltpu.make_async_copy(src, dst, first_sem.at[i]) for i, (src, dst) in enumerate((
        (wq_hbm.at[lo, left], wf.at[0, lo, left]),
        (x_hbm.at[pl.ds(0, 2), pl.ds(0, 64), lo], xf.at[0, pl.ds(0, 2), :, lo]),
        (wq_hbm.at[lo, right], wf.at[0, lo, right]),
        (wq_hbm.at[hi, pl.ds(0, 256)], wf.at[0, hi]),
        (x_hbm.at[pl.ds(0, 2), pl.ds(0, 64), hi], xf.at[0, pl.ds(0, 2), :, hi]),
        (x_hbm.at[pl.ds(2, 2), pl.ds(0, 64)], xf.at[0, pl.ds(2, 2)])))]
    for cp in first:
        cp.start()
    for i in range(1, 4):
        col_load(wq_hbm, wf, w_sem, i).start()
        x_load(i).start()

    table = _schedule()
    for i, row in enumerate(table):
        for j, word in enumerate(row):
            tab[ROW * i + j] = word

    def x_blocks(r, a):
        return [xf[r, 2 * h + a // 4, pl.ds(16 * (a % 4), 16), pl.ds(512 * b, 512)]
                for h in range(2) for b in range(2)]

    def wq_blocks(p, a):
        return [wf[p, pl.ds(512 * h + 64 * a, 64), pl.ds(128 * b, 128)] * Q_SCALE
                for h in range(2) for b in range(2)]

    def x_own(r, terms=True, send=(0, 1, 2, 3), slot=0):
        for a in range(8):
            blocks = x_blocks(r, a)
            for q in send:
                xs[slot, q, pl.ds(16 * a, 16), :] = blocks[q].astype(BF16)
            for j, term in enumerate(_lhs_terms(*blocks) if terms else ()):
                xc[j, r, pl.ds(16 * a, 16), :] = term.astype(BF16)

    def x_own_term(r, j):
        term = jnp.concatenate(
            [_lhs_terms(*x_blocks(r, a))[j].astype(BF16) for a in range(8)], axis=0)
        xc[j, r] = term
        return term

    def x_received(r, pieces):
        for a in pieces:
            rows = pl.ds(16 * a, 16)
            blocks = [xr[r, q, rows, :].astype(F32) for q in range(4)]
            for j, term in enumerate(_lhs_terms(*blocks)):
                xc[j, 4 + r, rows, :] = term.astype(BF16)

    def wq_own(p, terms=True, send=(0, 1, 2, 3)):
        for a in range(8):
            blocks = wq_blocks(p, a)
            for q in send:
                ws[p, q, pl.ds(64 * a, 64), :] = blocks[q].astype(BF16)
            for j, term in enumerate(_rhs_terms(*blocks) if terms else ()):
                wc[p, j, pl.ds(64 * a, 64), :] = term.astype(BF16)

    def wq_own_term(p, j):
        term = jnp.concatenate(
            [_rhs_terms(*wq_blocks(p, a))[j].astype(BF16) for a in range(8)], axis=0)
        wc[p, j] = term
        return term

    def received_term(buf, i, j):
        return jnp.concatenate(
            [_rhs_term(j, lambda q: buf[i, q, pl.ds(64 * a, 64), :]) for a in range(8)], axis=0)

    def wq_received(p, pieces):
        for a in pieces:
            rows = pl.ds(64 * a, 64)
            for j in range(7):
                wc[4 + p, j, rows, :] = _rhs_term(j, lambda q: wr[p, q, rows, :])

    def wo_own(c, slot, pieces):
        for a in pieces:
            rows = pl.ds(64 * a, 64)
            blocks = [wof[c, pl.ds(256 * (a // 2) + 128 * h + 64 * (a % 2), 64),
                          pl.ds(128 * b, 128)] for h in range(2) for b in range(2)]
            for q in range(4):
                wos[slot, q, rows, :] = blocks[q].astype(BF16)
            for j, term in enumerate(_rhs_terms(*blocks)):
                woc[slot, j, rows, :] = term.astype(BF16)

    def wo_received_term(c, j):
        woc[c, j, pl.ds(512, 512), :] = term = received_term(wor, c, j)
        return jnp.concatenate([woc[c, j, pl.ds(0, 512), :], term], axis=0)

    def unit(word, i):
        return (word >> (6 * i)) & 7, (word >> (6 * i + 3)) & 7

    def keys(pair, which, chunk):
        start = (chunk & 3) * 64
        return jnp.concatenate(
            [kvf[pair, which, pl.ds(pl.multiple_of(start + 256 * j, 64), 64), :] for j in range(4)],
            axis=0).astype(BF16)

    def scores(chunk, pair):
        return [lax.dot_general(qb[chunk, pair, b], keys(pair, b, chunk),
                                (((1,), (1,)), ((), ())), preferred_element_type=F32)
                for b in range(2)]

    def softmax(s):
        p = jnp.exp2(s - jnp.max(s, axis=1, keepdims=True))
        total = jnp.sum(p, axis=1, keepdims=True)
        inv = pl.reciprocal(total, approx=True)
        inv = inv * (2.0 - total * inv)
        return p.astype(BF16), inv

    def context(chunk, pair, probs):
        c0, c1 = [_dot(p, keys(pair, 2 + b, chunk)) * inv
                  for b, (p, inv) in enumerate(probs)]
        for j, term in enumerate(_lhs_terms(c0[:128], c1[:128], c0[128:], c1[128:])):
            cc[j, pair, chunk] = term.astype(BF16)

    def project(chunk, pair, lhs=None, rhs=None, after=None):
        count = iter(range(7))

        def prod(j):
            m = _dot(xc[j, chunk] if lhs is None else lhs(j),
                     wc[pair, j] if rhs is None else rhs(j))
            if after is not None:
                after(next(count))
            return m

        top, bottom = pl.ds(0, 128), pl.ds(128, 128)
        m2, m1, m3, m4 = prod(1), prod(0), prod(2), prod(3)
        qb[chunk, pair, 0, bottom, :] = (m2 + m4).astype(BF16)
        m5 = prod(4)
        qb[chunk, pair, 1, top, :] = (m3 + m5).astype(BF16)
        m6 = prod(5)
        qb[chunk, pair, 1, bottom, :] = (m1 - m2 + m3 + m6).astype(BF16)
        m7 = prod(6)
        qb[chunk, pair, 0, top, :] = (m1 + m4 - m5 + m7).astype(BF16)

    def attend(word):
        units = [unit(word, i) for i in range(4)]
        s, p = {}, {}
        for stage in "q0 q1 s0 v0 q2 s1 v1 q3 s2 v2 s3 v3".split():
            i = int(stage[1])
            if stage[0] == "q":
                s[i] = scores(*units[i])
            elif stage[0] == "s":
                p[i] = [softmax(v) for v in s[i]]
            else:
                context(*units[i], p[i])

    def out_quadrants(chunk0, c, emit, rhs=None, after=None):
        def prod(j):
            lhs = jnp.concatenate(
                [cc[j, p, pl.ds(chunk0, 2)].reshape(256, 128) for p in range(8)], axis=1)
            m = _dot(lhs, woc[c, j] if rhs is None else rhs(j))
            if after is not None and j in after:
                after[j]()
            return m

        _strassen(prod, emit)

    first[0].wait()
    ws[0, 0] = (wf[0, lo, left] * Q_SCALE).astype(BF16)
    pl.semaphore_wait(barrier, 2)
    w_send(0, lead, 4).start()
    first[1].wait()
    xs[0, 0] = xf[0, pl.ds(0, 2), :, lo].reshape(128, 512).astype(BF16)
    x_send(0, lead, 4).start()
    first[2].wait()
    first[3].wait()
    wq_own(0, send=(1, 2, 3))
    w_send(0, rest).start()
    first[4].wait()
    first[5].wait()
    x_own(0, send=(1, 2, 3))
    x_send(0, rest).start()


    def decode(i):
        head = tab[ROW * i]
        return (head & 15, head >> 4,
                tab[ROW * i + 1], tab[ROW * i + 2], tab[ROW * i + 3])

    def first_step(i, carry):
        kind, arg, _, proj, _ = decode(i)

        def step_qx():
            new, r = arg < 4, arg & 3

            @pl.when(new)
            def _():
                x_load(r).wait()

            project(*unit(proj, 0), lhs=lambda j: x_own_term(r, j))
            project(*unit(proj, 1),
                    after=lambda k: k == 0 and x_own(r, False, slot=jnp.minimum(arg, 4)))

            @pl.when(new)
            def _():
                x_send(r).start()

                @pl.when(arg > 1)
                def _():
                    kv_start(2 * arg - 4)

        def step_qw():
            col_load(wq_hbm, wf, w_sem, arg).wait()
            project(*unit(proj, 0), rhs=lambda j: wq_own_term(arg, j))
            project(*unit(proj, 1), after=lambda k: k == 0 and wq_own(arg, False))
            w_send(arg).start()

            @pl.when(arg == 3)
            def _():
                kv_start(1)

        _switch(kind, FIRST_KINDS, dict(QX=step_qx, QW=step_qw))
        return carry

    def step(i, carry):
        kind, arg, kv, proj, attn = decode(i)

        def with_keys(work):
            def run():
                @pl.when((kv & 15) != 0)
                def _():
                    kv_wait((kv & 15) - 1)

                work()

                @pl.when(kv >= 16)
                def _():
                    kv_start(kv >> 4)
            return run

        def project_and_attend(extra=()):
            work = [[] for _ in range(7 * 4 + 1)]
            for u in range(4):
                a_unit, state = unit(attn, u), {}

                def qk(a_unit=a_unit, state=state):
                    state["s"] = scores(*a_unit)

                def sm(state=state):
                    state["p"] = [softmax(v) for v in state["s"]]

                def pv(a_unit=a_unit, state=state):
                    context(*a_unit, state["p"])

                for ahead, stage in zip(ATTN_AT, (qk, sm, pv)):
                    work[min(7 * u + ahead, 26)].append(stage)
            for g, job in extra:
                work[g].append(job)
            for job in work[0]:
                job()
            for u in range(4):
                project(*unit(proj, u),
                        after=lambda k, u=u: [job() for job in work[7 * u + k + 1]])

        def step_sj():
            col_load(wo_hbm, wof, wo_sem, arg - 1).wait()
            w_send(arg).wait_recv()
            x_send(arg).wait_recv()
            col_load(wo_hbm, wof, wo_sem, arg).start()
            jobs = dict(w=lambda a: wq_received(arg, (a,)), x=lambda a: x_received(arg, (a,)),
                        o=lambda a: wo_own(arg - 1, arg - 1, (a,)))
            project_and_attend([
                (7 * u + k + 1, lambda v=v: jobs[v[0]](int(v[1])))
                for u in range(4) for k, work in enumerate(SIDE_WORK[u].split("|"))
                for v in work.split()])
            wo_send(arg - 1).start()

        def step_ox():
            @pl.when(arg == 0)
            def _():
                col_load(wo_hbm, wof, wo_sem, 3).wait()

            wo_send(arg).wait_recv()
            sends = p_sends(arg)
            slot = jnp.where(arg == 0, 3, 4)
            spare = {j: lambda a=a: wo_own(3, slot, (a, a + 1))
                     for j, a in zip((2, 4, 0, 5), range(0, 8, 2))}
            for t in range(2):
                def emit(part, half, tile, val, t=t):
                    ps[2 * arg + t, part] = val.astype(BF16)

                out_quadrants(4 + 2 * t, arg, emit,
                              rhs=(lambda j: wo_received_term(arg, j)) if t == 0 else None,
                              after={2 - t: sends[t].start, **(spare if t else {})})
            sends[2].start()

            @pl.when(arg == 0)
            def _():
                wo_send(3).start()

        def step_oo():
            filled = set()
            for j, uses in USES:
                def prod(i, j=j):
                    def left(q):
                        return jnp.concatenate(
                            [cc[j, 4 * (q % 2) + p, pl.ds(2 * (q // 2), 2)].reshape(256, 128)
                             for p in range(4)], axis=1)

                    def right(q):
                        return woc[2 * arg + q % 2, j, pl.ds(512 * (q // 2), 512), :]

                    return _dot(_lhs_term(i, left), _rhs_term(i, right))

                def add(_, t, c, val, uses=uses):
                    for half, tile, sign in uses:
                        at = (t, c, half, tile)
                        if at in filled:
                            acc[at] = acc[at] + val if sign > 0 else acc[at] - val
                        else:
                            acc[at] = val if sign > 0 else -val
                            filled.add(at)

                _strassen(prod, add)

            for c, t, half, tile in sorted((c, t, h, n) for t, c, h, n in filled):
                if (half, tile) == (0, 0):
                    copies = p_sends(2 * arg + c)
                    for cp in copies[2:] if t else copies[:2]:
                        cp.wait_recv()
                part = {(1, 0): 0, (0, 1): 1, (1, 1): 2, (0, 0): 3}[half, tile]
                val = acc[t, c, half, tile] + pr[2 * (2 * arg + c) + t, part].astype(F32)
                val = val.astype(BF16)
                cols = pl.ds(pl.multiple_of((2 * arg + c) * 256 + 128 * tile, 128), 128)
                for chunk in range(2):
                    for blk in range(2):
                        row = 256 * (2 * half + blk) + 64 * (2 * t + chunk)
                        src = 128 * chunk + 64 * blk
                        out_ref[0, pl.ds(row, 64), cols] = val[src:src + 64]

        def step_qj():
            col_load(wo_hbm, wof, wo_sem, 0).start()
            for send in (w_send, x_send):
                send(0, lead, 4).wait_recv()
                send(0, rest).wait_recv()
            project(*unit(proj, 0),
                    after=lambda k: wq_received(arg, (k,) if k < 6 else (6, 7)))
            project(*unit(proj, 1),
                    after=lambda k: x_received(arg, (k + 1,) if k else (0, 1)))

        _switch(kind, KINDS, dict(
            S=with_keys(project_and_attend), SJ=with_keys(step_sj),
            A=with_keys(lambda: attend(attn)),
            OX=step_ox, OO=step_oo, QJ=step_qj))
        return carry

    lax.fori_loop(0, 7, first_step, 0)
    lax.fori_loop(7, len(table), step, 0)

    for stream, buf in enumerate((xs.at[pl.ds(0, 4)], ws, wos.at[pl.ds(0, 4)], ps)):
        pltpu.make_async_remote_copy(
            buf, buf, send_sem.at[stream], xr_sem.at[0],
            device_id=(me,), device_id_type=pl.DeviceIdType.MESH).wait_send()


def pallas_dist_sparse_attn_strided_qseq_b1_sq1024_skv1024_hq8_dh128_kernel(
    x: jax.Array,
    Wq: jax.Array,
    K_ext: jax.Array,
    V_ext: jax.Array,
    Wo: jax.Array,
):
    dma = pltpu.SemaphoreType.DMA
    scratch = [
        pltpu.VMEM((4, 4, 64, 1024), F32),
        pltpu.VMEM((4, 1024, 256), F32),
        pltpu.VMEM((4, 1024, 256), F32),
        pltpu.VMEM((8, 4, 1024, 128), F32),
        pltpu.VMEM((5, 4, 128, 512), BF16),
        pltpu.VMEM((4, 4, 128, 512), BF16),
        pltpu.VMEM((4, 4, 512, 128), BF16),
        pltpu.VMEM((4, 4, 512, 128), BF16),
        pltpu.VMEM((5, 4, 512, 128), BF16),
        pltpu.VMEM((4, 4, 512, 128), BF16),
        pltpu.VMEM((8, 4, 256, 128), BF16),
        pltpu.VMEM((8, 4, 256, 128), BF16),
        pltpu.VMEM((7, 8, 128, 512), BF16),
        pltpu.VMEM((8, 7, 512, 128), BF16),
        pltpu.VMEM((5, 7, 1024, 128), BF16),
        pltpu.VMEM((8, 8, 2, 256, 128), BF16),
        pltpu.VMEM((7, 8, 8, 128, 128), BF16),
        pltpu.VMEM((2, 2, 2, 2, 256, 128), F32),
        pltpu.SMEM((ROW * len(_schedule()),), jnp.int32),
        dma((4,)), dma((4,)), dma((4,)), dma((8,)), dma((6,)),
        dma((4,)), dma((5,)), dma((5,)), dma((4,)), dma((12,)),
    ]
    return pl.pallas_call(
        _body,
        out_shape=jax.ShapeDtypeStruct((1, 1024, 1024), BF16),
        in_specs=[pl.BlockSpec(memory_space=pltpu.MemorySpace.HBM)] * 5,
        out_specs=pl.BlockSpec(memory_space=pltpu.MemorySpace.VMEM),
        scratch_shapes=scratch,
        compiler_params=pltpu.CompilerParams(
            collective_id=0, vmem_limit_bytes=120 * 1024 * 1024,
            disable_bounds_checks=True, disable_semaphore_checks=True),
    )(x.reshape(4, 256, 1024), Wq, K_ext.reshape(1024, 32, 128),
      V_ext.reshape(1024, 32, 128), Wo)
```
